```python
import numpy as np

kernel_name = "dist_layernorm_xy_m6144_n2048"

def setup_inputs():
    x = np.random.randn(12288, 4096).astype(np.float32)
    gamma = np.random.randn(4096).astype(np.float32)
    beta = np.random.randn(4096).astype(np.float32)
    return {"x": x, "gamma": gamma, "beta": beta}

def reference(x: np.ndarray, gamma: np.ndarray, beta: np.ndarray) -> np.ndarray:
    eps = 1e-5
    mean = np.mean(x, axis=1, keepdims=True)
    var = np.var(x, axis=1, keepdims=True)
    return gamma * (x - mean) / np.sqrt(var + eps) + beta
```

```python
import jax
import jax.numpy as jnp
from jax import lax
from jax.experimental import pallas as pl
from jax.experimental.pallas import tpu as pltpu

EPS = 1e-5
LANES = 128
CH = 128
PHASES = ((4, 10), (2, 3), (1, 2))
D = 4
L = 1


def pallas_dist_layernorm_xy_m6144_n2048_kernel(
    x: jax.Array,
    gamma: jax.Array,
    beta: jax.Array,
):
    M, N = x.shape
    NG = 2 * N
    NT = N // LANES
    G = CH // 8
    SEG = LANES // G
    nc = M // CH
    ph = []
    s = 0
    base = 0
    for z, n in PHASES:
        ph.append((s, s + z * n, z, base))
        s += z * n
        base += n
    nb = base
    assert s == nc

    def body(x_hbm, g_hbm, b_hbm, o_ref,
             xbuf, gb_in, gb8, st_send, st_recv,
             rsem, gsem, ssem, vsem):
        my_x = lax.axis_index("x")
        my_y = lax.axis_index("y")
        nbr = (my_x, 1 - my_y)
        bar = pltpu.get_barrier_semaphore()
        pl.semaphore_signal(bar, inc=1, device_id=nbr, device_id_type=pl.DeviceIdType.MESH)

        gcopy = pltpu.make_async_copy(g_hbm, gb_in.at[pl.ds(0, 1)], gsem.at[0])
        bcopy = pltpu.make_async_copy(b_hbm, gb_in.at[pl.ds(8, 1)], gsem.at[1])

        def rd(p, bl):
            s0, e0, z, b0 = ph[p]
            r0 = (s0 + bl * z) * CH
            if not isinstance(r0, int):
                r0 = pl.multiple_of(r0, CH)
            return pltpu.make_async_copy(x_hbm.at[pl.ds(r0, z * CH)], xbuf.at[pl.ds(r0, z * CH)], rsem.at[b0 + bl])

        def start_reads_at(c):
            cc = c + D
            for p, (s0, e0, z, b0) in enumerate(ph):
                if isinstance(c, int):
                    if s0 <= cc < e0 and (cc - s0) % z == 0:
                        rd(p, (cc - s0) // z).start()
                else:
                    @pl.when((cc >= s0) & (cc < e0) & ((cc - s0) % z == 0))
                    def _(p=p, s0=s0, z=z):
                        rd(p, (cc - s0) // z).start()

        def wait_reads_at(c):
            for p, (s0, e0, z, b0) in enumerate(ph):
                if isinstance(c, int):
                    if s0 <= c < e0 and (c - s0) % z == 0:
                        rd(p, (c - s0) // z).wait()
                else:
                    @pl.when((c >= s0) & (c < e0) & ((c - s0) % z == 0))
                    def _(p=p, s0=s0, z=z):
                        rd(p, (c - s0) // z).wait()

        for c in range(-D, 0):
            start_reads_at(c)
        gcopy.start()
        bcopy.start()

        def rcopy(c):
            r0 = c * 16
            if not isinstance(r0, int):
                r0 = pl.multiple_of(r0, 16)
            return pltpu.make_async_remote_copy(
                src_ref=st_send.at[pl.ds(r0, 16)], dst_ref=st_recv.at[pl.ds(r0, 16)],
                send_sem=ssem.at[c], recv_sem=vsem.at[c],
                device_id=nbr, device_id_type=pl.DeviceIdType.MESH)

        lane = lax.broadcasted_iota(jnp.int32, (8, LANES), 1)
        seg = lane // SEG
        nlev = G.bit_length() - 1
        masks = [((seg >> b) & 1) == 1 for b in range(nlev)]

        def compact(vals):
            cur = list(vals)
            for b in range(nlev):
                cur = [jnp.where(masks[b], cur[2 * i + 1], cur[2 * i]) for i in range(len(cur) // 2)]
            return cur[0]

        def tree_sum(ts, nacc=4):
            acc = [None] * nacc
            for i, t in enumerate(ts):
                acc[i % nacc] = t if acc[i % nacc] is None else acc[i % nacc] + t
            while len(acc) > 1:
                acc = [acc[2 * i] + acc[2 * i + 1] for i in range(len(acc) // 2)]
            return acc[0]

        def stats_chunk(c):
            r0 = c * CH
            means, m2s = [], []
            for g in range(G):
                rr = r0 + 8 * g
                if not isinstance(rr, int):
                    rr = pl.multiple_of(rr, 8)
                xs = [xbuf[pl.ds(rr, 8), t * LANES:(t + 1) * LANES] for t in range(NT)]
                mean = jnp.sum(tree_sum(xs), axis=1, keepdims=True) * (1.0 / N)
                mean = jnp.broadcast_to(mean, (8, LANES))
                ds = [xv - mean for xv in xs]
                m2 = jnp.sum(tree_sum([d * d for d in ds]), axis=1, keepdims=True)
                means.append(mean)
                m2s.append(jnp.broadcast_to(m2, (8, LANES)))
            s0 = c * 16
            if not isinstance(s0, int):
                s0 = pl.multiple_of(s0, 16)
            st_send[pl.ds(s0, 8), :] = compact(means)
            st_send[pl.ds(s0 + 8, 8), :] = compact(m2s)

        def norm_chunk(c):
            r0 = c * CH
            s0 = c * 16
            if not isinstance(s0, int):
                s0 = pl.multiple_of(s0, 16)
            a_l = st_send[pl.ds(s0, 8), :]
            b_l = st_send[pl.ds(s0 + 8, 8), :]
            a_r = st_recv[pl.ds(s0, 8), :]
            b_r = st_recv[pl.ds(s0 + 8, 8), :]
            mean_c = (a_l + a_r) * 0.5
            dm = a_l - a_r
            m2 = (b_l + b_r) + dm * dm * (N / 2.0)
            rstd_c = lax.rsqrt(m2 * (1.0 / NG) + EPS)

            def bcast(t, g):
                k = g * SEG
                return jnp.broadcast_to(t[:, k:k + 1], (8, LANES))

            for p in range(G // 2):
                rr = r0 + 16 * p
                if not isinstance(rr, int):
                    rr = pl.multiple_of(rr, 16)
                mean = jnp.concatenate([bcast(mean_c, 2 * p), bcast(mean_c, 2 * p + 1)], axis=0)
                rstd = jnp.concatenate([bcast(rstd_c, 2 * p), bcast(rstd_c, 2 * p + 1)], axis=0)
                for t in range(NT):
                    xt = xbuf[pl.ds(rr, 16), t * LANES:(t + 1) * LANES]
                    gt = gb8[0:16, t * LANES:(t + 1) * LANES]
                    bt = gb8[16:32, t * LANES:(t + 1) * LANES]
                    y = ((xt - mean) * rstd) * gt + bt
                    o_ref[pl.ds(rr, 16), t * LANES:(t + 1) * LANES] = y.astype(jnp.bfloat16)

        def front(c, first=False):
            start_reads_at(c)
            wait_reads_at(c)
            stats_chunk(c)
            if first:
                pl.semaphore_wait(bar, 1)
            rcopy(c).start()

        def back(j):
            rcopy(j).wait_recv()
            norm_chunk(j)

        front(0, first=True)
        gcopy.wait()
        bcopy.wait()
        gb8[0:16, :] = jnp.broadcast_to(gb_in[0:1, :], (16, N))
        gb8[16:32, :] = jnp.broadcast_to(gb_in[8:9, :], (16, N))

        def loop_body(c, _):
            front(c)

            @pl.when(c >= L)
            def _():
                back(c - L)
            return 0
        lax.fori_loop(1, nc, loop_body, 0)

        def epi(j, _):
            back(j)
            return 0
        lax.fori_loop(nc - L, nc, epi, 0)

        def wsend(c, _):
            rcopy(c).wait_send()
            return 0
        lax.fori_loop(0, nc, wsend, 0)

    return pl.pallas_call(
        body,
        out_shape=pltpu.VMEM((M, N), jnp.bfloat16),
        in_specs=[pl.BlockSpec(memory_space=pl.ANY)] * 3,
        out_specs=pl.BlockSpec(memory_space=pltpu.VMEM),
        scratch_shapes=[
            pltpu.VMEM((M, N), jnp.float32),
            pltpu.VMEM((16, N), jnp.float32),
            pltpu.VMEM((32, N), jnp.float32),
            pltpu.VMEM((nc * 16, LANES), jnp.float32),
            pltpu.VMEM((nc * 16, LANES), jnp.float32),
            pltpu.SemaphoreType.DMA((nb,)),
            pltpu.SemaphoreType.DMA((2,)),
            pltpu.SemaphoreType.DMA((nc,)),
            pltpu.SemaphoreType.DMA((nc,)),
        ],
        compiler_params=pltpu.CompilerParams(
            collective_id=0, vmem_limit_bytes=64 * 1024 * 1024, disable_semaphore_checks=True),
    )(x, gamma.reshape(1, N), beta.reshape(1, N))
```

```python
import jax
import jax.numpy as jnp
from jax import lax
from jax.experimental import pallas as pl
from jax.experimental.pallas import tpu as pltpu

EPS = 1e-5
LANES = 128
SUB = 8
CH = 128
K = 2


def _tree_sum(terms, nacc=4):
    acc = [None] * nacc
    for i, t in enumerate(terms):
        acc[i % nacc] = t if acc[i % nacc] is None else acc[i % nacc] + t
    while len(acc) > 1:
        acc = [acc[2 * i] + acc[2 * i + 1] for i in range(len(acc) // 2)]
    return acc[0]


def pallas_dist_layernorm_xy_m6144_n2048_kernel(
    x: jax.Array,
    gamma: jax.Array,
    beta: jax.Array,
):
    M, N = x.shape
    NG = 2 * N
    NT = N // LANES
    G = CH // SUB
    SEG = LANES // G
    nc = M // CH
    assert M % CH == 0 and N % LANES == 0 and nc > K

    def body(x_hbm, g_hbm, b_hbm, o_ref,
             xbuf, gb_in, gb, st_send, st_recv,
             rd_sem, gb_sem, send_sem, recv_sem):
        my_x = lax.axis_index("x")
        my_y = lax.axis_index("y")
        nbr = (my_x, 1 - my_y)

        barrier = pltpu.get_barrier_semaphore()
        pl.semaphore_signal(barrier, inc=1, device_id=nbr,
                            device_id_type=pl.DeviceIdType.MESH)

        def read(c):
            r0 = c * CH
            if not isinstance(r0, int):
                r0 = pl.multiple_of(r0, CH)
            return pltpu.make_async_copy(
                x_hbm.at[pl.ds(r0, CH)], xbuf.at[pl.ds(r0, CH)], rd_sem.at[c])

        def stats_slot(c):
            s0 = c * 2 * SUB
            return s0 if isinstance(s0, int) else pl.multiple_of(s0, 2 * SUB)

        def exchange(c):
            s0 = stats_slot(c)
            return pltpu.make_async_remote_copy(
                src_ref=st_send.at[pl.ds(s0, 2 * SUB)],
                dst_ref=st_recv.at[pl.ds(s0, 2 * SUB)],
                send_sem=send_sem, recv_sem=recv_sem.at[c],
                device_id=nbr, device_id_type=pl.DeviceIdType.MESH)

        gamma_copy = pltpu.make_async_copy(g_hbm, gb_in.at[pl.ds(0, 1)], gb_sem.at[0])
        beta_copy = pltpu.make_async_copy(b_hbm, gb_in.at[pl.ds(SUB, 1)], gb_sem.at[1])

        for c in range(K):
            read(c).start()
        gamma_copy.start()
        beta_copy.start()

        lane = lax.broadcasted_iota(jnp.int32, (SUB, LANES), 1)

        def pack(vals):
            cur = list(vals)
            bit = SEG.bit_length() - 1
            while len(cur) > 1:
                m = ((lane >> bit) & 1) == 1
                cur = [jnp.where(m, cur[2 * i + 1], cur[2 * i]) for i in range(len(cur) // 2)]
                bit += 1
            return cur[0]

        def stats(c):
            r0 = c * CH
            means, m2s = [], []
            for g in range(G):
                rr = r0 + SUB * g
                if not isinstance(rr, int):
                    rr = pl.multiple_of(rr, SUB)
                xs = [xbuf[pl.ds(rr, SUB), t * LANES:(t + 1) * LANES] for t in range(NT)]
                mean = jnp.sum(_tree_sum(xs), axis=1, keepdims=True) * (1.0 / N)
                mean = jnp.broadcast_to(mean, (SUB, LANES))
                ds = [xv - mean for xv in xs]
                m2 = jnp.sum(_tree_sum([d * d for d in ds]), axis=1, keepdims=True)
                means.append(mean)
                m2s.append(jnp.broadcast_to(m2, (SUB, LANES)))
            s0 = stats_slot(c)
            st_send[pl.ds(s0, SUB), :] = pack(means)
            st_send[pl.ds(s0 + SUB, SUB), :] = pack(m2s)

        def normalise(c):
            r0 = c * CH
            s0 = stats_slot(c)
            mean_l = st_send[pl.ds(s0, SUB), :]
            m2_l = st_send[pl.ds(s0 + SUB, SUB), :]
            mean_r = st_recv[pl.ds(s0, SUB), :]
            m2_r = st_recv[pl.ds(s0 + SUB, SUB), :]
            mean_c = (mean_l + mean_r) * 0.5
            dm = mean_l - mean_r
            m2 = (m2_l + m2_r) + dm * dm * (N / 2.0)
            rstd_c = lax.rsqrt(m2 * (1.0 / NG) + EPS)

            def unpack(t, g):
                k = g * SEG
                return jnp.broadcast_to(t[:, k:k + 1], (SUB, LANES))

            for p in range(G // 2):
                rr = r0 + 2 * SUB * p
                if not isinstance(rr, int):
                    rr = pl.multiple_of(rr, 2 * SUB)
                mean = jnp.concatenate([unpack(mean_c, 2 * p), unpack(mean_c, 2 * p + 1)], axis=0)
                rstd = jnp.concatenate([unpack(rstd_c, 2 * p), unpack(rstd_c, 2 * p + 1)], axis=0)
                for t in range(NT):
                    cols = slice(t * LANES, (t + 1) * LANES)
                    xt = xbuf[pl.ds(rr, 2 * SUB), cols]
                    y = ((xt - mean) * rstd) * gb[0:2 * SUB, cols] + gb[2 * SUB:4 * SUB, cols]
                    o_ref[pl.ds(rr, 2 * SUB), cols] = y.astype(o_ref.dtype)

        def front(c, first=False):
            read(c).wait()
            if isinstance(c, int):
                if c + K < nc:
                    read(c + K).start()
            else:
                @pl.when(c + K < nc)
                def _():
                    read(c + K).start()
            stats(c)
            if first:
                pl.semaphore_wait(barrier, 1)
            exchange(c).start()

        def back(c):
            exchange(c).wait_recv()
            normalise(c)

        front(0, first=True)
        gamma_copy.wait()
        beta_copy.wait()
        gb[0:2 * SUB, :] = jnp.broadcast_to(gb_in[0:1, :], (2 * SUB, N))
        gb[2 * SUB:4 * SUB, :] = jnp.broadcast_to(gb_in[SUB:SUB + 1, :], (2 * SUB, N))

        def step(c, carry):
            front(c)
            back(c - 1)
            return carry

        lax.fori_loop(1, nc, step, 0)
        back(nc - 1)

        pltpu.make_async_remote_copy(
            src_ref=st_send, dst_ref=st_recv, send_sem=send_sem, recv_sem=recv_sem.at[0],
            device_id=nbr, device_id_type=pl.DeviceIdType.MESH).wait_send()

    return pl.pallas_call(
        body,
        out_shape=pltpu.VMEM((M, N), jnp.bfloat16),
        in_specs=[pl.BlockSpec(memory_space=pl.ANY)] * 3,
        out_specs=pl.BlockSpec(memory_space=pltpu.VMEM),
        scratch_shapes=[
            pltpu.VMEM((M, N), jnp.float32),
            pltpu.VMEM((2 * SUB, N), jnp.float32),
            pltpu.VMEM((4 * SUB, N), jnp.float32),
            pltpu.VMEM((nc * 2 * SUB, LANES), jnp.float32),
            pltpu.VMEM((nc * 2 * SUB, LANES), jnp.float32),
            pltpu.SemaphoreType.DMA((nc,)),
            pltpu.SemaphoreType.DMA((2,)),
            pltpu.SemaphoreType.DMA,
            pltpu.SemaphoreType.DMA((nc,)),
        ],
        compiler_params=pltpu.CompilerParams(
            collective_id=0,
            vmem_limit_bytes=64 * 1024 * 1024,
            disable_semaphore_checks=True,
        ),
    )(x, gamma.reshape(1, N), beta.reshape(1, N))
```

```python
import jax
import jax.numpy as jnp
from jax import lax
from jax.experimental import pallas as pl
from jax.experimental.pallas import tpu as pltpu

EPS = 1e-5
LANES = 128
SUB = 8
CH = 128
K = 2


def _tree_sum(terms, nacc=4):
    acc = [None] * nacc
    for i, t in enumerate(terms):
        acc[i % nacc] = t if acc[i % nacc] is None else acc[i % nacc] + t
    while len(acc) > 1:
        acc = [acc[2 * i] + acc[2 * i + 1] for i in range(len(acc) // 2)]
    return acc[0]


def pallas_dist_layernorm_xy_m6144_n2048_kernel(
    x: jax.Array,
    gamma: jax.Array,
    beta: jax.Array,
):
    M, N = x.shape
    NG = 2 * N
    NT = N // LANES
    G = CH // SUB
    SEG = LANES // G
    nc = M // CH
    assert M % CH == 0 and N % LANES == 0 and nc > K

    def body(x_hbm, g_hbm, b_hbm, o_ref,
             xbuf, gb_in, gb, st_send, st_recv,
             rd_sem, gb_sem, send_sem, recv_sem):
        my_x = lax.axis_index("x")
        my_y = lax.axis_index("y")
        nbr = (my_x, 1 - my_y)

        barrier = pltpu.get_barrier_semaphore()
        pl.semaphore_signal(barrier, inc=1, device_id=nbr,
                            device_id_type=pl.DeviceIdType.MESH)

        def read(c):
            r0 = c * CH
            if not isinstance(r0, int):
                r0 = pl.multiple_of(r0, CH)
            return pltpu.make_async_copy(
                x_hbm.at[pl.ds(r0, CH)], xbuf.at[pl.ds(r0, CH)], rd_sem.at[c])

        def stats_slot(c):
            s0 = c * 2 * SUB
            return s0 if isinstance(s0, int) else pl.multiple_of(s0, 2 * SUB)

        def exchange(c):
            s0 = stats_slot(c)
            return pltpu.make_async_remote_copy(
                src_ref=st_send.at[pl.ds(s0, 2 * SUB)],
                dst_ref=st_recv.at[pl.ds(s0, 2 * SUB)],
                send_sem=send_sem, recv_sem=recv_sem.at[c],
                device_id=nbr, device_id_type=pl.DeviceIdType.MESH)

        gamma_copy = pltpu.make_async_copy(g_hbm, gb_in.at[pl.ds(0, 1)], gb_sem.at[0])
        beta_copy = pltpu.make_async_copy(b_hbm, gb_in.at[pl.ds(SUB, 1)], gb_sem.at[1])

        for c in range(K):
            read(c).start()
        gamma_copy.start()
        beta_copy.start()

        lane = lax.broadcasted_iota(jnp.int32, (SUB, LANES), 1)

        def pack(vals):
            cur = list(vals)
            bit = SEG.bit_length() - 1
            while len(cur) > 1:
                m = ((lane >> bit) & 1) == 1
                cur = [jnp.where(m, cur[2 * i + 1], cur[2 * i]) for i in range(len(cur) // 2)]
                bit += 1
            return cur[0]

        def stats(c):
            r0 = c * CH
            means, m2s = [], []
            for g in range(G):
                rr = r0 + SUB * g
                if not isinstance(rr, int):
                    rr = pl.multiple_of(rr, SUB)
                xs = [xbuf[pl.ds(rr, SUB), t * LANES:(t + 1) * LANES] for t in range(NT)]
                mean = jnp.sum(_tree_sum(xs), axis=1, keepdims=True) * (1.0 / N)
                mean = jnp.broadcast_to(mean, (SUB, LANES))
                ds = [xv - mean for xv in xs]
                m2 = jnp.sum(_tree_sum([d * d for d in ds]), axis=1, keepdims=True)
                means.append(mean)
                m2s.append(jnp.broadcast_to(m2, (SUB, LANES)))
            s0 = stats_slot(c)
            st_send[pl.ds(s0, SUB), :] = pack(means)
            st_send[pl.ds(s0 + SUB, SUB), :] = pack(m2s)

        def normalise(c):
            r0 = c * CH
            s0 = stats_slot(c)
            mean_l = st_send[pl.ds(s0, SUB), :]
            m2_l = st_send[pl.ds(s0 + SUB, SUB), :]
            mean_r = st_recv[pl.ds(s0, SUB), :]
            m2_r = st_recv[pl.ds(s0 + SUB, SUB), :]
            mean_c = (mean_l + mean_r) * 0.5
            dm = mean_l - mean_r
            m2 = (m2_l + m2_r) + dm * dm * (N / 2.0)
            rstd_c = lax.rsqrt(m2 * (1.0 / NG) + EPS)

            def unpack(t, g):
                k = g * SEG
                return jnp.broadcast_to(t[:, k:k + 1], (SUB, LANES))

            for p in range(G // 2):
                rr = r0 + 2 * SUB * p
                if not isinstance(rr, int):
                    rr = pl.multiple_of(rr, 2 * SUB)
                means = [unpack(mean_c, 2 * p), unpack(mean_c, 2 * p + 1)]
                rstds = [unpack(rstd_c, 2 * p), unpack(rstd_c, 2 * p + 1)]
                for t in range(NT):
                    cols = slice(t * LANES, (t + 1) * LANES)
                    gt = gb[0:SUB, cols]
                    bt = gb[SUB:2 * SUB, cols]
                    ys = []
                    for h in range(2):
                        xt = xbuf[pl.ds(pl.multiple_of(rr + SUB * h, SUB), SUB), cols]
                        ys.append(((xt - means[h]) * rstds[h]) * gt + bt)
                    o_ref[pl.ds(rr, 2 * SUB), cols] = jnp.concatenate(ys, axis=0).astype(o_ref.dtype)

        def front(c, first=False):
            read(c).wait()
            if isinstance(c, int):
                if c + K < nc:
                    read(c + K).start()
            else:
                @pl.when(c + K < nc)
                def _():
                    read(c + K).start()
            stats(c)
            if first:
                pl.semaphore_wait(barrier, 1)
            exchange(c).start()

        def back(c):
            exchange(c).wait_recv()
            normalise(c)

        front(0, first=True)
        gamma_copy.wait()
        beta_copy.wait()
        gb[0:SUB, :] = jnp.broadcast_to(gb_in[0:1, :], (SUB, N))
        gb[SUB:2 * SUB, :] = jnp.broadcast_to(gb_in[SUB:SUB + 1, :], (SUB, N))

        def step(c, carry):
            front(c)
            back(c - 1)
            return carry

        lax.fori_loop(1, nc, step, 0)
        back(nc - 1)

        pltpu.make_async_remote_copy(
            src_ref=st_send, dst_ref=st_recv, send_sem=send_sem, recv_sem=recv_sem.at[0],
            device_id=nbr, device_id_type=pl.DeviceIdType.MESH).wait_send()

    return pl.pallas_call(
        body,
        out_shape=pltpu.VMEM((M, N), jnp.bfloat16),
        in_specs=[pl.BlockSpec(memory_space=pl.ANY)] * 3,
        out_specs=pl.BlockSpec(memory_space=pltpu.VMEM),
        scratch_shapes=[
            pltpu.VMEM((M, N), jnp.float32),
            pltpu.VMEM((2 * SUB, N), jnp.float32),
            pltpu.VMEM((2 * SUB, N), jnp.float32),
            pltpu.VMEM((nc * 2 * SUB, LANES), jnp.float32),
            pltpu.VMEM((nc * 2 * SUB, LANES), jnp.float32),
            pltpu.SemaphoreType.DMA((nc,)),
            pltpu.SemaphoreType.DMA((2,)),
            pltpu.SemaphoreType.DMA,
            pltpu.SemaphoreType.DMA((nc,)),
        ],
        compiler_params=pltpu.CompilerParams(
            collective_id=0,
            vmem_limit_bytes=64 * 1024 * 1024,
            disable_semaphore_checks=True,
        ),
    )(x, gamma.reshape(1, N), beta.reshape(1, N))
```

```python
import jax
import jax.numpy as jnp
from jax import lax
from jax.experimental import pallas as pl
from jax.experimental.pallas import tpu as pltpu

EPS = 1e-5
LANES = 128
SUB = 8
CH = 128
TAIL = (96, 32)
K = len(TAIL)


def _aligned(v, k):
    return v if isinstance(v, int) else pl.multiple_of(v, k)


def _pow2_at_least(n):
    p = 1
    while p < n:
        p *= 2
    return p


def _tree_sum(terms, nacc=4):
    acc = [None] * nacc
    for i, t in enumerate(terms):
        acc[i % nacc] = t if acc[i % nacc] is None else acc[i % nacc] + t
    while len(acc) > 1:
        acc = [acc[2 * i] + acc[2 * i + 1] for i in range(len(acc) // 2)]
    return acc[0]


def pallas_dist_layernorm_xy_m6144_n2048_kernel(
    x: jax.Array,
    gamma: jax.Array,
    beta: jax.Array,
):
    M, N = x.shape
    NG = 2 * N
    NT = N // LANES
    n_main = (M - sum(TAIL)) // CH
    assert n_main * CH + sum(TAIL) == M and N % LANES == 0 and n_main > K
    assert all(t % (2 * SUB) == 0 and t <= CH for t in TAIL)
    chunk_rows = [CH] * n_main + list(TAIL)
    chunk_row0 = [sum(chunk_rows[:c]) for c in range(len(chunk_rows))]
    nc = len(chunk_rows)
    MSG = 2 * SUB

    def body(x_hbm, g_hbm, b_hbm, o_ref,
             xbuf, gb_in, gb, st_send, st_recv,
             rd_sem, gb_sem, send_sem, recv_sem):
        my_x = lax.axis_index("x")
        my_y = lax.axis_index("y")
        nbr = (my_x, 1 - my_y)

        barrier = pltpu.get_barrier_semaphore()
        pl.semaphore_signal(barrier, inc=1, device_id=nbr,
                            device_id_type=pl.DeviceIdType.MESH)

        def geometry(c):
            if isinstance(c, int):
                return chunk_row0[c], chunk_rows[c]
            return pl.multiple_of(c * CH, CH), CH

        def read(c):
            r0, nr = geometry(c)
            return pltpu.make_async_copy(
                x_hbm.at[pl.ds(r0, nr)], xbuf.at[pl.ds(r0, nr)], rd_sem.at[c])

        def exchange(c):
            s0 = _aligned(c * MSG, MSG)
            return pltpu.make_async_remote_copy(
                src_ref=st_send.at[pl.ds(s0, MSG)],
                dst_ref=st_recv.at[pl.ds(s0, MSG)],
                send_sem=send_sem, recv_sem=recv_sem.at[c],
                device_id=nbr, device_id_type=pl.DeviceIdType.MESH)

        gamma_copy = pltpu.make_async_copy(g_hbm, gb_in.at[pl.ds(0, 1)], gb_sem.at[0])
        beta_copy = pltpu.make_async_copy(b_hbm, gb_in.at[pl.ds(SUB, 1)], gb_sem.at[1])

        for c in range(K):
            read(c).start()
        gamma_copy.start()
        beta_copy.start()

        lane = lax.broadcasted_iota(jnp.int32, (SUB, LANES), 1)

        def pack(vals):
            cur = list(vals) + [vals[-1]] * (_pow2_at_least(len(vals)) - len(vals))
            bit = (LANES // len(cur)).bit_length() - 1
            while len(cur) > 1:
                m = ((lane >> bit) & 1) == 1
                cur = [jnp.where(m, cur[2 * i + 1], cur[2 * i]) for i in range(len(cur) // 2)]
                bit += 1
            return cur[0]

        def stats(c):
            r0, nr = geometry(c)
            means, m2s = [], []
            for g in range(nr // SUB):
                rr = _aligned(r0 + SUB * g, SUB)
                xs = [xbuf[pl.ds(rr, SUB), t * LANES:(t + 1) * LANES] for t in range(NT)]
                mean = jnp.sum(_tree_sum(xs), axis=1, keepdims=True) * (1.0 / N)
                mean = jnp.broadcast_to(mean, (SUB, LANES))
                ds = [xv - mean for xv in xs]
                m2 = jnp.sum(_tree_sum([d * d for d in ds]), axis=1, keepdims=True)
                means.append(mean)
                m2s.append(jnp.broadcast_to(m2, (SUB, LANES)))
            s0 = _aligned(c * MSG, MSG)
            st_send[pl.ds(s0, SUB), :] = pack(means)
            st_send[pl.ds(s0 + SUB, SUB), :] = pack(m2s)

        def normalise(c):
            r0, nr = geometry(c)
            groups = nr // SUB
            seg = LANES // _pow2_at_least(groups)
            s0 = _aligned(c * MSG, MSG)
            mean_l = st_send[pl.ds(s0, SUB), :]
            m2_l = st_send[pl.ds(s0 + SUB, SUB), :]
            mean_r = st_recv[pl.ds(s0, SUB), :]
            m2_r = st_recv[pl.ds(s0 + SUB, SUB), :]
            mean_c = (mean_l + mean_r) * 0.5
            dm = mean_l - mean_r
            m2 = (m2_l + m2_r) + dm * dm * (N / 2.0)
            rstd_c = lax.rsqrt(m2 * (1.0 / NG) + EPS)

            def unpack(t, g):
                k = g * seg
                return jnp.broadcast_to(t[:, k:k + 1], (SUB, LANES))

            for p in range(groups // 2):
                rr = _aligned(r0 + 2 * SUB * p, 2 * SUB)
                means = [unpack(mean_c, 2 * p), unpack(mean_c, 2 * p + 1)]
                rstds = [unpack(rstd_c, 2 * p), unpack(rstd_c, 2 * p + 1)]
                for t in range(NT):
                    cols = slice(t * LANES, (t + 1) * LANES)
                    gt = gb[0:SUB, cols]
                    bt = gb[SUB:2 * SUB, cols]
                    ys = []
                    for h in range(2):
                        xt = xbuf[pl.ds(_aligned(rr + SUB * h, SUB), SUB), cols]
                        ys.append(((xt - means[h]) * rstds[h]) * gt + bt)
                    o_ref[pl.ds(rr, 2 * SUB), cols] = jnp.concatenate(ys, axis=0).astype(o_ref.dtype)

        def front(c, first=False):
            read(c).wait()
            if isinstance(c, int):
                if c + K < n_main:
                    read(c + K).start()
            else:
                @pl.when(c + K < n_main)
                def _():
                    read(c + K).start()
                for j in range(K):
                    @pl.when(c == n_main - K + j)
                    def _(j=j):
                        read(n_main + j).start()
            stats(c)
            if first:
                pl.semaphore_wait(barrier, 1)
            exchange(c).start()

        def back(c):
            exchange(c).wait_recv()
            normalise(c)

        front(0, first=True)
        gamma_copy.wait()
        beta_copy.wait()
        gb[0:SUB, :] = jnp.broadcast_to(gb_in[0:1, :], (SUB, N))
        gb[SUB:2 * SUB, :] = jnp.broadcast_to(gb_in[SUB:SUB + 1, :], (SUB, N))

        def step(c, carry):
            front(c)
            back(c - 1)
            return carry

        lax.fori_loop(1, n_main, step, 0)
        for c in range(n_main, nc):
            front(c)
        for c in range(n_main - 1, nc):
            back(c)

        pltpu.make_async_remote_copy(
            src_ref=st_send, dst_ref=st_recv, send_sem=send_sem, recv_sem=recv_sem.at[0],
            device_id=nbr, device_id_type=pl.DeviceIdType.MESH).wait_send()

    return pl.pallas_call(
        body,
        out_shape=pltpu.VMEM((M, N), jnp.bfloat16),
        in_specs=[pl.BlockSpec(memory_space=pl.ANY)] * 3,
        out_specs=pl.BlockSpec(memory_space=pltpu.VMEM),
        scratch_shapes=[
            pltpu.VMEM((M, N), jnp.float32),
            pltpu.VMEM((2 * SUB, N), jnp.float32),
            pltpu.VMEM((2 * SUB, N), jnp.float32),
            pltpu.VMEM((nc * MSG, LANES), jnp.float32),
            pltpu.VMEM((nc * MSG, LANES), jnp.float32),
            pltpu.SemaphoreType.DMA((nc,)),
            pltpu.SemaphoreType.DMA((2,)),
            pltpu.SemaphoreType.DMA,
            pltpu.SemaphoreType.DMA((nc,)),
        ],
        compiler_params=pltpu.CompilerParams(
            collective_id=0,
            vmem_limit_bytes=64 * 1024 * 1024,
            disable_semaphore_checks=True,
        ),
    )(x, gamma.reshape(1, N), beta.reshape(1, N))
```

```python
import jax
import jax.numpy as jnp
from jax import lax
from jax.experimental import pallas as pl
from jax.experimental.pallas import tpu as pltpu

EPS = 1e-5
LANES = 128
SUB = 8
CH = 128
TAIL = (96, 32)
K = len(TAIL)


def _aligned(v, k):
    return v if isinstance(v, int) else pl.multiple_of(v, k)


def _pow2_at_least(n):
    p = 1
    while p < n:
        p *= 2
    return p


def _tree_sum(terms, nacc=4):
    acc = [None] * nacc
    for i, t in enumerate(terms):
        acc[i % nacc] = t if acc[i % nacc] is None else acc[i % nacc] + t
    while len(acc) > 1:
        acc = [acc[2 * i] + acc[2 * i + 1] for i in range(len(acc) // 2)]
    return acc[0]


def pallas_dist_layernorm_xy_m6144_n2048_kernel(
    x: jax.Array,
    gamma: jax.Array,
    beta: jax.Array,
):
    M, N = x.shape
    NG = 2 * N
    NT = N // LANES
    n_main = (M - sum(TAIL)) // CH
    assert n_main * CH + sum(TAIL) == M and N % LANES == 0 and n_main > K
    assert all(t % (2 * SUB) == 0 and t <= CH for t in TAIL)
    chunk_rows = [CH] * n_main + list(TAIL)
    chunk_row0 = [sum(chunk_rows[:c]) for c in range(len(chunk_rows))]
    nc = len(chunk_rows)
    MSG = 2 * SUB

    def body(x_hbm, g_hbm, b_hbm, o_ref,
             xbuf, gb_in, gb, st_send, st_recv,
             rd_sem, gb_sem, send_sem, recv_sem):
        my_x = lax.axis_index("x")
        my_y = lax.axis_index("y")
        nbr = (my_x, 1 - my_y)

        barrier = pltpu.get_barrier_semaphore()
        pl.semaphore_signal(barrier, inc=1, device_id=nbr,
                            device_id_type=pl.DeviceIdType.MESH)

        def geometry(c):
            if isinstance(c, int):
                return chunk_row0[c], chunk_rows[c]
            return pl.multiple_of(c * CH, CH), CH

        def read(c):
            r0, nr = geometry(c)
            return pltpu.make_async_copy(
                x_hbm.at[pl.ds(r0, nr)], xbuf.at[pl.ds(r0, nr)], rd_sem.at[c])

        def exchange(c):
            s0 = _aligned(c * MSG, MSG)
            return pltpu.make_async_remote_copy(
                src_ref=st_send.at[pl.ds(s0, MSG)],
                dst_ref=st_recv.at[pl.ds(s0, MSG)],
                send_sem=send_sem.at[c], recv_sem=recv_sem.at[c],
                device_id=nbr, device_id_type=pl.DeviceIdType.MESH)

        gamma_copy = pltpu.make_async_copy(g_hbm, gb_in.at[pl.ds(0, 1)], gb_sem.at[0])
        beta_copy = pltpu.make_async_copy(b_hbm, gb_in.at[pl.ds(SUB, 1)], gb_sem.at[1])

        for c in range(K):
            read(c).start()
        gamma_copy.start()
        beta_copy.start()

        lane = lax.broadcasted_iota(jnp.int32, (SUB, LANES), 1)

        def pack(vals):
            cur = list(vals) + [vals[-1]] * (_pow2_at_least(len(vals)) - len(vals))
            bit = (LANES // len(cur)).bit_length() - 1
            while len(cur) > 1:
                m = ((lane >> bit) & 1) == 1
                cur = [jnp.where(m, cur[2 * i + 1], cur[2 * i]) for i in range(len(cur) // 2)]
                bit += 1
            return cur[0]

        def stats(c):
            r0, nr = geometry(c)
            means, m2s = [], []
            for g in range(nr // SUB):
                rr = _aligned(r0 + SUB * g, SUB)
                xs = [xbuf[pl.ds(rr, SUB), t * LANES:(t + 1) * LANES] for t in range(NT)]
                mean = jnp.sum(_tree_sum(xs), axis=1, keepdims=True) * (1.0 / N)
                mean = jnp.broadcast_to(mean, (SUB, LANES))
                ds = [xv - mean for xv in xs]
                m2 = jnp.sum(_tree_sum([d * d for d in ds]), axis=1, keepdims=True)
                means.append(mean)
                m2s.append(jnp.broadcast_to(m2, (SUB, LANES)))
            s0 = _aligned(c * MSG, MSG)
            st_send[pl.ds(s0, SUB), :] = pack(means)
            st_send[pl.ds(s0 + SUB, SUB), :] = pack(m2s)

        def normalise(c):
            r0, nr = geometry(c)
            groups = nr // SUB
            seg = LANES // _pow2_at_least(groups)
            s0 = _aligned(c * MSG, MSG)
            mean_l = st_send[pl.ds(s0, SUB), :]
            m2_l = st_send[pl.ds(s0 + SUB, SUB), :]
            mean_r = st_recv[pl.ds(s0, SUB), :]
            m2_r = st_recv[pl.ds(s0 + SUB, SUB), :]
            mean_c = (mean_l + mean_r) * 0.5
            dm = mean_l - mean_r
            m2 = (m2_l + m2_r) + dm * dm * (N / 2.0)
            rstd_c = lax.rsqrt(m2 * (1.0 / NG) + EPS)

            def unpack(t, g):
                k = g * seg
                return jnp.broadcast_to(t[:, k:k + 1], (SUB, LANES))

            for p in range(groups // 2):
                rr = _aligned(r0 + 2 * SUB * p, 2 * SUB)
                means = [unpack(mean_c, 2 * p), unpack(mean_c, 2 * p + 1)]
                rstds = [unpack(rstd_c, 2 * p), unpack(rstd_c, 2 * p + 1)]
                for t in range(NT):
                    cols = slice(t * LANES, (t + 1) * LANES)
                    gt = gb[0:SUB, cols]
                    bt = gb[SUB:2 * SUB, cols]
                    ys = []
                    for h in range(2):
                        xt = xbuf[pl.ds(_aligned(rr + SUB * h, SUB), SUB), cols]
                        ys.append(((xt - means[h]) * rstds[h]) * gt + bt)
                    o_ref[pl.ds(rr, 2 * SUB), cols] = jnp.concatenate(ys, axis=0).astype(o_ref.dtype)

        def front(c, first=False):
            read(c).wait()
            if isinstance(c, int):
                if c + K < n_main:
                    read(c + K).start()
            else:
                @pl.when(c + K < n_main)
                def _():
                    read(c + K).start()
                for j in range(K):
                    @pl.when(c == n_main - K + j)
                    def _(j=j):
                        read(n_main + j).start()
            stats(c)
            if first:
                pl.semaphore_wait(barrier, 1)
            exchange(c).start()

        def back(c):
            exchange(c).wait_recv()
            normalise(c)
            exchange(c).wait_send()

        front(0, first=True)
        gamma_copy.wait()
        beta_copy.wait()
        gb[0:SUB, :] = jnp.broadcast_to(gb_in[0:1, :], (SUB, N))
        gb[SUB:2 * SUB, :] = jnp.broadcast_to(gb_in[SUB:SUB + 1, :], (SUB, N))

        def step(c, carry):
            front(c)
            back(c - 1)
            return carry

        lax.fori_loop(1, n_main, step, 0)
        for c in range(n_main, nc):
            front(c)
        for c in range(n_main - 1, nc):
            back(c)

    return pl.pallas_call(
        body,
        out_shape=pltpu.VMEM((M, N), jnp.bfloat16),
        in_specs=[pl.BlockSpec(memory_space=pl.ANY)] * 3,
        out_specs=pl.BlockSpec(memory_space=pltpu.VMEM),
        scratch_shapes=[
            pltpu.VMEM((M, N), jnp.float32),
            pltpu.VMEM((2 * SUB, N), jnp.float32),
            pltpu.VMEM((2 * SUB, N), jnp.float32),
            pltpu.VMEM((nc * MSG, LANES), jnp.float32),
            pltpu.VMEM((nc * MSG, LANES), jnp.float32),
            pltpu.SemaphoreType.DMA((nc,)),
            pltpu.SemaphoreType.DMA((2,)),
            pltpu.SemaphoreType.DMA((nc,)),
            pltpu.SemaphoreType.DMA((nc,)),
        ],
        compiler_params=pltpu.CompilerParams(
            collective_id=0,
            vmem_limit_bytes=64 * 1024 * 1024,
            disable_semaphore_checks=True,
        ),
    )(x, gamma.reshape(1, N), beta.reshape(1, N))
```
